```python
import numpy as np

kernel_name = "dist_argmax_global_i_m8192_n1024"

def setup_inputs():
    return {"x": np.random.randn(32768, 1024).astype(np.float32)}

def reference(x: np.ndarray) -> np.ndarray:
    idx = np.argmax(x, axis=0).astype(np.float32)
    val = np.max(x, axis=0)
    return np.stack([val, idx], axis=0)
```

```python
import jax
import jax.numpy as jnp
from jax import lax
from jax.experimental import pallas as pl
from jax.experimental.pallas import tpu as pltpu

M, N = 8192, 1024
ND = 4
NB = N // 128
MESH = pl.DeviceIdType.MESH

PIECES = (128, 128, 128)
PIECE_AT = (4, 8, 12)
MERGE_AT = 14
CHUNKS = (512,) * 13 + (256,) + (256, 128, 64, 32, 16, 8, 8)
UNROLL = 4
F = sum(PIECES)


def _merge(ev, ei, lv, li):
    idx = jnp.where(lv <= ev, ei, jnp.where(ev != ev, ei, li))
    return jnp.maximum(ev, lv), idx


def _scan(ref, r0, nrows, rowbase, acc):
    ng = nrows // 8
    u = min(UNROLL, ng)
    while ng % u:
        u -= 1
    sub = lax.broadcasted_iota(jnp.int32, (8, 128), 0)

    def step(t, acc):
        vs, ids = list(acc[0]), list(acc[1])
        for k in range(u):
            g = t * u + k
            r = r0 + g * 8
            if not isinstance(r, int):
                r = pl.multiple_of(r, 8)
            rowv = sub + (rowbase + g * 8)
            for c in range(NB):
                xv = ref[pl.ds(r, 8), c * 128:(c + 1) * 128]
                vs[c], ids[c] = _merge(vs[c], ids[c], xv, rowv)
        return tuple(vs), tuple(ids)

    if ng // u == 1:
        return step(0, acc)
    return lax.fori_loop(0, ng // u, step, acc)


def _init_acc():
    return (tuple(jnp.full((8, 128), -jnp.inf, jnp.float32) for _ in range(NB)),
            tuple(jnp.zeros((8, 128), jnp.int32) for _ in range(NB)))


def _reduce_store(acc, dst):
    vs, ids = acc
    for c in range(NB):
        mx = jnp.max(vs[c], axis=0, keepdims=True)
        hit = jnp.logical_or(vs[c] == mx, vs[c] != vs[c])
        ix = jnp.min(jnp.where(hit, ids[c], jnp.int32(2**30)), axis=0, keepdims=True)
        dst[0:1, c * 128:(c + 1) * 128] = mx
        dst[1:2, c * 128:(c + 1) * 128] = ix.astype(jnp.float32)


def pallas_dist_argmax_global_i_m8192_n1024_kernel(x):
    assert x.shape == (M, N) and sum(CHUNKS) == M - 2 * F
    offs = [2 * F + sum(CHUNKS[:i]) for i in range(len(CHUNKS))]
    poffs = [sum(PIECES[:i]) for i in range(len(PIECES))]
    nc, npc = len(CHUNKS), len(PIECES)

    def body(x_hbm, out_ref, buf, sems, gath, ssem, rsem, raw, raw_ssem, raw_rsem,
             pout, pin, p_ssem, p_rsem, ready, accv, acci):
        me = lax.axis_index("i")
        right = (me + 1) % ND
        left = (me + ND - 1) % ND

        def cp(i):
            return pltpu.make_async_copy(
                x_hbm.at[pl.ds(offs[i], CHUNKS[i]), :],
                buf.at[pl.ds(offs[i] - 2 * F, CHUNKS[i]), :], sems.at[i])

        for i in range(nc):
            cp(i).start()

        bar = pltpu.get_barrier_semaphore()
        for nb in (left, right):
            pl.semaphore_signal(bar, inc=1, device_id=(nb,), device_id_type=MESH)
        pl.semaphore_wait(bar, 2)
        for nb in (left, right):
            pl.semaphore_signal(ready, inc=1, device_id=(nb,), device_id_type=MESH)

        def rawcp(d, p):
            return pltpu.make_async_remote_copy(
                x_hbm.at[pl.ds(d * F + poffs[p], PIECES[p]), :],
                raw.at[d, pl.ds(poffs[p], PIECES[p]), :],
                raw_ssem.at[d, p], raw_rsem.at[d, p],
                device_id=((right if d == 0 else left),), device_id_type=MESH)

        for p in range(npc):
            for d in range(2):
                rawcp(d, p).start()

        def pcp(d):
            return pltpu.make_async_remote_copy(
                pout.at[d], pin.at[d], p_ssem.at[d], p_rsem.at[d],
                device_id=((left if d == 0 else right),), device_id_type=MESH)

        acc = _init_acc()
        for i in range(nc):
            cp(i).wait()
            acc = _scan(buf, offs[i] - 2 * F, CHUNKS[i], me * M + offs[i], acc)
            for p in range(npc):
                if PIECE_AT[p] != i:
                    continue
                for d in range(2):
                    rawcp(d, p).wait_recv()
                    owner = left if d == 0 else right
                    if p == 0:
                        a = _init_acc()
                    else:
                        a = (tuple(accv[d, c] for c in range(NB)),
                             tuple(acci[d, c] for c in range(NB)))
                    a = _scan(raw.at[d], poffs[p], PIECES[p],
                              owner * M + d * F + poffs[p], a)
                    if p < npc - 1:
                        for c in range(NB):
                            accv[d, c] = a[0][c]
                            acci[d, c] = a[1][c]
                    else:
                        _reduce_store(a, pout.at[d])
                        pcp(d).start()
            if MERGE_AT == i:
                pl.semaphore_wait(ready, 2)
                for d in range(2):
                    pcp(d).wait_recv()
                vs, ids = list(acc[0]), list(acc[1])
                for c in range(NB):
                    sl = slice(c * 128, (c + 1) * 128)
                    sv, si = _merge(pin[0, 0:1, sl], pin[0, 1:2, sl],
                                    pin[1, 0:1, sl], pin[1, 1:2, sl])
                    sv = jnp.broadcast_to(sv, (8, 128))
                    si = jnp.broadcast_to(si.astype(jnp.int32), (8, 128))
                    vs[c], ids[c] = _merge(sv, si, vs[c], ids[c])
                acc = (tuple(vs), tuple(ids))

        def gcp(slot, d, dev):
            return pltpu.make_async_remote_copy(
                gath.at[slot], gath.at[slot], ssem.at[d - 1], rsem.at[d - 1],
                device_id=(dev,), device_id_type=MESH)

        _reduce_store(acc, gath.at[me])
        sends = []
        for d in (2, 1, 3):
            c = gcp(me, d, (me + d) % ND)
            c.start()
            sends.append(c)
        for d in (1, 3, 2):
            src = (me + ND - d) % ND
            gcp(src, d, src).wait_recv()
        bv, bi = gath[0, 0:1, :], gath[0, 1:2, :]
        for k in range(1, ND):
            bv, bi = _merge(bv, bi, gath[k, 0:1, :], gath[k, 1:2, :])
        out_ref[0:1, :] = bv
        out_ref[1:2, :] = bi
        for c in sends:
            c.wait_send()
        for p in range(npc):
            for d in range(2):
                rawcp(d, p).wait_send()
        for d in range(2):
            pcp(d).wait_send()

    return pl.pallas_call(
        body,
        out_shape=jax.ShapeDtypeStruct((2, N), jnp.float32),
        in_specs=[pl.BlockSpec(memory_space=pl.ANY)],
        out_specs=pl.BlockSpec(memory_space=pltpu.VMEM),
        scratch_shapes=[
            pltpu.VMEM((M - 2 * F, N), jnp.float32),
            pltpu.SemaphoreType.DMA((nc,)),
            pltpu.VMEM((ND, 2, N), jnp.float32),
            pltpu.SemaphoreType.DMA((ND - 1,)),
            pltpu.SemaphoreType.DMA((ND - 1,)),
            pltpu.VMEM((2, F, N), jnp.float32),
            pltpu.SemaphoreType.DMA((2, npc)),
            pltpu.SemaphoreType.DMA((2, npc)),
            pltpu.VMEM((2, 2, N), jnp.float32),
            pltpu.VMEM((2, 2, N), jnp.float32),
            pltpu.SemaphoreType.DMA((2,)),
            pltpu.SemaphoreType.DMA((2,)),
            pltpu.SemaphoreType.REGULAR,
            pltpu.VMEM((2, NB, 8, 128), jnp.float32),
            pltpu.VMEM((2, NB, 8, 128), jnp.int32),
        ],
        compiler_params=pltpu.CompilerParams(
            vmem_limit_bytes=48 * 1024 * 1024, collective_id=0,
            disable_bounds_checks=True, disable_semaphore_checks=True),
    )(x)
```

```python
import jax
import jax.numpy as jnp
from jax import lax
from jax.experimental import pallas as pl
from jax.experimental.pallas import tpu as pltpu

M, N = 8192, 1024
ND = 4
LANES = 128
SUB = 8
NB = N // LANES
MESH = pl.DeviceIdType.MESH

PIECES = (128, 128, 128, 64)
CHUNKS = (512,) * 6 + (96,) + (512,) * 3 + (96,) + (512,) * 3 + (288, 256, 128, 128)
VIA_SMEM = {6: 3, 10: 5}
PIECE_AT = (4, 9, 13, 14)
MERGE_AT = 16
TAIL = 160
GROUPS = (4, 2, 1, 1)
UNROLL = 4

F = sum(PIECES)


def _merge(ev, ei, lv, li):
    idx = jnp.where(lv <= ev, ei, jnp.where(ev != ev, ei, li))
    return jnp.maximum(ev, lv), idx


def _block(c):
    return slice(c * LANES, (c + 1) * LANES)


def _init_acc():
    return (tuple(jnp.full((SUB, LANES), -jnp.inf, jnp.float32) for _ in range(NB)),
            tuple(jnp.zeros((SUB, LANES), jnp.int32) for _ in range(NB)))


def _scan(ref, r0, nrows, row_id0, acc):
    ng = nrows // SUB
    u = min(UNROLL, ng)
    while ng % u:
        u -= 1
    sub = lax.broadcasted_iota(jnp.int32, (SUB, LANES), 0)

    def step(t, acc):
        vs, ids = list(acc[0]), list(acc[1])
        for k in range(u):
            g = t * u + k
            r = r0 + g * SUB
            if not isinstance(r, int):
                r = pl.multiple_of(r, SUB)
            rows = sub + (row_id0 + g * SUB)
            for c in range(NB):
                vs[c], ids[c] = _merge(vs[c], ids[c], ref[pl.ds(r, SUB), _block(c)], rows)
        return tuple(vs), tuple(ids)

    if ng == u:
        return step(0, acc)
    return lax.fori_loop(0, ng // u, step, acc)


def _scan_tree(ref, r0, nrows, row_id0, acc, cols):
    vs, ids = list(acc[0]), list(acc[1])
    sub = lax.broadcasted_iota(jnp.int32, (SUB, LANES), 0)
    rows = [sub + (row_id0 + g * SUB) for g in range(nrows // SUB)]
    for c in cols:
        items = [(ref[pl.ds(r0 + g * SUB, SUB), _block(c)], rows[g])
                 for g in range(nrows // SUB)]
        while len(items) > 1:
            nxt = [_merge(*items[j], *items[j + 1]) for j in range(0, len(items) - 1, 2)]
            items = nxt + items[len(items) - len(items) % 2:]
        vs[c], ids[c] = _merge(vs[c], ids[c], *items[0])
    return tuple(vs), tuple(ids)


def _reduce_store(acc, dst, cols):
    vs, ids = acc
    for c in cols:
        mx = jnp.max(vs[c], axis=0, keepdims=True)
        hit = jnp.logical_or(vs[c] == mx, vs[c] != vs[c])
        ix = jnp.min(jnp.where(hit, ids[c], jnp.int32(2**30)), axis=0, keepdims=True)
        dst[0:1, _block(c)] = mx
        dst[1:2, _block(c)] = ix.astype(jnp.float32)


def pallas_dist_argmax_global_i_m8192_n1024_kernel(x):
    assert x.shape == (M, N)
    nc, npc, ngr = len(CHUNKS), len(PIECES), len(GROUPS)
    assert 2 * F + sum(CHUNKS) + TAIL == M and sum(GROUPS) == NB
    offs = [2 * F + sum(CHUNKS[:i]) for i in range(nc)]
    poffs = [sum(PIECES[:p]) for p in range(npc)]
    soffs, srows = {}, 0
    for i in sorted(VIA_SMEM):
        soffs[i] = srows
        srows += CHUNKS[i]
    tail0 = M - TAIL
    gcols = [range(sum(GROUPS[:g]), sum(GROUPS[:g + 1])) for g in range(ngr)]

    def body(x_hbm, out_ref, buf, csem, tsem, sbuf, ssem, raw, raw_ssem, raw_rsem,
             accv, acci, pout, pin, p_ssem, p_rsem, ready, gath, g_ssem, g_rsem):
        me = lax.axis_index("i")
        right = (me + 1) % ND
        left = (me + ND - 1) % ND

        def lanes(g):
            return pl.ds(gcols[g][0] * LANES, GROUPS[g] * LANES)

        def chunk_cp(i):
            src = (sbuf.at[pl.ds(soffs[i], CHUNKS[i]), :] if i in VIA_SMEM
                   else x_hbm.at[pl.ds(offs[i], CHUNKS[i]), :])
            return pltpu.make_async_copy(
                src, buf.at[pl.ds(offs[i] - 2 * F, CHUNKS[i]), :], csem.at[i])

        def smem_cp(i):
            return pltpu.make_async_copy(
                x_hbm.at[pl.ds(offs[i], CHUNKS[i]), :],
                sbuf.at[pl.ds(soffs[i], CHUNKS[i]), :],
                ssem.at[sorted(VIA_SMEM).index(i)])

        def tail_cp(g):
            return pltpu.make_async_copy(
                x_hbm.at[pl.ds(tail0, TAIL), lanes(g)],
                buf.at[pl.ds(tail0 - 2 * F, TAIL), lanes(g)], tsem.at[g])

        def raw_cp(d, p):
            return pltpu.make_async_remote_copy(
                x_hbm.at[pl.ds(d * F + poffs[p], PIECES[p]), :],
                raw.at[d, pl.ds(poffs[p], PIECES[p]), :],
                raw_ssem.at[d, p], raw_rsem.at[d, p],
                device_id=(right if d == 0 else left,), device_id_type=MESH)

        def part_cp(d):
            return pltpu.make_async_remote_copy(
                pout.at[d], pin.at[d], p_ssem.at[d], p_rsem.at[d],
                device_id=(left if d == 0 else right,), device_id_type=MESH)

        def gath_cp(slot, d, g):
            return pltpu.make_async_remote_copy(
                gath.at[slot, :, lanes(g)], gath.at[slot, :, lanes(g)],
                g_ssem.at[d - 1, g], g_rsem.at[d - 1, g],
                device_id=((me + d) % ND,), device_id_type=MESH)

        for i in range(nc):
            if i not in VIA_SMEM:
                chunk_cp(i).start()
        for g in range(ngr):
            tail_cp(g).start()
        for i in sorted(VIA_SMEM):
            smem_cp(i).start()

        barrier = pltpu.get_barrier_semaphore()
        for nb in (left, right):
            pl.semaphore_signal(barrier, inc=1, device_id=(nb,), device_id_type=MESH)
        pl.semaphore_wait(barrier, 2)
        for nb in (left, right):
            pl.semaphore_signal(ready, inc=1, device_id=(nb,), device_id_type=MESH)
        for p in range(npc):
            for d in range(2):
                raw_cp(d, p).start()

        acc = _init_acc()
        for i in range(nc):
            chunk_cp(i).wait()
            acc = _scan(buf, offs[i] - 2 * F, CHUNKS[i], me * M + offs[i], acc)
            for j, at in VIA_SMEM.items():
                if at == i:
                    smem_cp(j).wait()
                    chunk_cp(j).start()
            if i in PIECE_AT:
                p = PIECE_AT.index(i)
                for d in range(2):
                    raw_cp(d, p).wait_recv()
                    if p == 0:
                        a = _init_acc()
                    else:
                        a = (tuple(accv[d, c] for c in range(NB)),
                             tuple(acci[d, c] for c in range(NB)))
                    owner = left if d == 0 else right
                    a = _scan(raw.at[d], poffs[p], PIECES[p],
                              owner * M + d * F + poffs[p], a)
                    if p < npc - 1:
                        for c in range(NB):
                            accv[d, c] = a[0][c]
                            acci[d, c] = a[1][c]
                    else:
                        _reduce_store(a, pout.at[d], range(NB))
                        part_cp(d).start()
            if i == MERGE_AT:
                pl.semaphore_wait(ready, 2)
                for d in range(2):
                    part_cp(d).wait_recv()
                vs, ids = list(acc[0]), list(acc[1])
                for c in range(NB):
                    hv, hi = _merge(pin[0, 0:1, _block(c)], pin[0, 1:2, _block(c)],
                                    pin[1, 0:1, _block(c)], pin[1, 1:2, _block(c)])
                    hv = jnp.broadcast_to(hv, (SUB, LANES))
                    hi = jnp.broadcast_to(hi.astype(jnp.int32), (SUB, LANES))
                    vs[c], ids[c] = _merge(hv, hi, vs[c], ids[c])
                acc = (tuple(vs), tuple(ids))

        for g in range(ngr):
            tail_cp(g).wait()
            acc = _scan_tree(buf, tail0 - 2 * F, TAIL, me * M + tail0, acc, gcols[g])
            _reduce_store(acc, gath.at[me], gcols[g])
            for d in (2, 1, 3):
                gath_cp(me, d, g).start()

        for p in range(npc):
            for d in range(2):
                raw_cp(d, p).wait_send()
        for d in range(2):
            part_cp(d).wait_send()
        for g in range(ngr):
            for d in range(1, ND):
                gath_cp(me, d, g).wait_send()

        for g in range(ngr):
            for d in (1, 3, 2):
                gath_cp((me + ND - d) % ND, d, g).wait_recv()
            sl = slice(gcols[g][0] * LANES, (gcols[g][-1] + 1) * LANES)
            bv, bi = gath[0, 0:1, sl], gath[0, 1:2, sl]
            for k in range(1, ND):
                bv, bi = _merge(bv, bi, gath[k, 0:1, sl], gath[k, 1:2, sl])
            out_ref[0:1, sl] = bv
            out_ref[1:2, sl] = bi

    dma = pltpu.SemaphoreType.DMA
    return pl.pallas_call(
        body,
        out_shape=jax.ShapeDtypeStruct((2, N), jnp.float32),
        in_specs=[pl.BlockSpec(memory_space=pl.ANY)],
        out_specs=pl.BlockSpec(memory_space=pltpu.VMEM),
        scratch_shapes=[
            pltpu.VMEM((M - 2 * F, N), jnp.float32),
            dma((nc,)),
            dma((ngr,)),
            pltpu.SMEM((srows, N), jnp.float32),
            dma((len(VIA_SMEM),)),
            pltpu.VMEM((2, F, N), jnp.float32),
            dma((2, npc)),
            dma((2, npc)),
            pltpu.VMEM((2, NB, SUB, LANES), jnp.float32),
            pltpu.VMEM((2, NB, SUB, LANES), jnp.int32),
            pltpu.VMEM((2, 2, N), jnp.float32),
            pltpu.VMEM((2, 2, N), jnp.float32),
            dma((2,)),
            dma((2,)),
            pltpu.SemaphoreType.REGULAR,
            pltpu.VMEM((ND, 2, N), jnp.float32),
            dma((ND - 1, ngr)),
            dma((ND - 1, ngr)),
        ],
        compiler_params=pltpu.CompilerParams(
            vmem_limit_bytes=48 * 1024 * 1024,
            collective_id=0,
            disable_bounds_checks=True,
            disable_semaphore_checks=True,
        ),
    )(x)
```
